```python
import numpy as np

kernel_name = "dist_halo_stencil_i_m8192_n1024"

def setup_inputs():
    return {"x": np.random.randn(32768, 1024).astype(np.float32)}

def reference(x: np.ndarray) -> np.ndarray:
    out = np.empty_like(x)
    out[0] = x[0]
    out[-1] = x[-1]
    out[1:-1] = 0.25 * x[:-2] + 0.5 * x[1:-1] + 0.25 * x[2:]
    return out
```

```python
import jax
import jax.numpy as jnp
from jax import lax
from jax.experimental import pallas as pl
from jax.experimental.pallas import tpu as pltpu

N_DEV = 4
M, N = 8192, 1024
SUB, LANE = 8, 128
NC = N // LANE
A = 128
R = M // A
TILES = R // SUB * NC
PITCH = SUB * (TILES + 1)

PIECES = ((56, 64, 0, 8),) + tuple((r, r + 8, 0, 8) for r in range(0, 48, 8)) + (
    (48, 56, 0, 4), (48, 56, 4, 7), (48, 56, 7, 8))
HALO_AFTER = 3


def _off(r):
    return SUB * NC * (r // SUB) + r % SUB


def _body(x_hbm, k_ref, xb, carry, read_sems, send_sems, recv_sems):
    b4 = xb.reshape(A + 2, TILES + 1, SUB, LANE)
    reads = []
    for i, (r0, r1, c0, c1) in enumerate(PIECES):
        t = pl.ds(NC * (r0 // SUB) + c0, NC * ((r1 - r0) // SUB - 1) + c1 - c0)
        reads.append(pltpu.make_async_copy(x_hbm.at[:, t], b4.at[pl.ds(1, A), t], read_sems.at[i]))
    for c in reads:
        c.start()

    me = lax.axis_index("i")
    left = (me + N_DEV - 1) % N_DEV
    right = (me + 1) % N_DEV
    barrier = pltpu.get_barrier_semaphore()
    for nb in (left, right):
        pl.semaphore_signal(barrier, inc=1, device_id=(nb,), device_id_type=pl.DeviceIdType.MESH)
    first, last = pl.ds(0, NC), pl.ds(TILES - NC, NC)
    up = pltpu.make_async_remote_copy(
        b4.at[1, first], b4.at[A + 1, first], send_sems.at[0], recv_sems.at[0],
        device_id=(left,), device_id_type=pl.DeviceIdType.MESH)
    down = pltpu.make_async_remote_copy(
        b4.at[A, last], b4.at[0, last], send_sems.at[1], recv_sems.at[1],
        device_id=(right,), device_id_type=pl.DeviceIdType.MESH)

    have = [set() for _ in range(NC)]
    todo = [set(range(R)) for _ in range(NC)]

    def process(new, c0, c1):
        for cc in range(c0, c1):
            have[cc] |= set(new)
            outs = sorted(r for r in todo[cc] if {r - 1, r, r + 1} <= have[cc])
            todo[cc] -= set(outs)
            keep = [r for r in new if {r - 1, r, r + 1} & todo[cc]]

        def job(cc):
            sh = SUB * cc
            t = {r: xb[pl.ds(PITCH * (1 + r // R) + _off(r % R) + sh, A, stride=PITCH), :].T for r in new}

            def get(r):
                if r not in t:
                    t[r] = carry[_off(r) + sh]
                return t[r]

            for r in outs:
                c = get(r)
                v = (0.25 * get(r - 1) + 0.5 * c) + 0.25 * get(r + 1)
                if r in (0, R - 1):
                    a = lax.broadcasted_iota(jnp.int32, (LANE, A), 1)
                    edge = (a == 0) & (me == 0) if r == 0 else (a == A - 1) & (me == N_DEV - 1)
                    v = jnp.where(edge, c, v)
                k_ref[_off(r) + sh] = v
            for r in keep:
                carry[_off(r) + sh] = t[r]

        if c1 - c0 == 1:
            job(c0)
        else:
            pl.loop(c0, c1)(job)

    for i, (r0, r1, c0, c1) in enumerate(PIECES):
        reads[i].wait()
        if i == 0:
            pl.semaphore_wait(barrier, 2)
        if r1 == R:
            down.start()
        if r0 == 0:
            up.start()
        process(list(range(r0, r1)), c0, c1)
        if i == HALO_AFTER:
            up.wait_recv()
            down.wait_recv()
            process([-1, R], 0, NC)
            up.wait_send()
            down.wait_send()


def pallas_dist_halo_stencil_i_m8192_n1024_kernel(x: jax.Array):
    xv = x.reshape(M // SUB, SUB, NC, LANE).transpose(0, 2, 1, 3).reshape(A, TILES, SUB, LANE)
    k = pl.pallas_call(
        _body,
        out_shape=pltpu.VMEM((TILES * SUB, LANE, A), x.dtype),
        in_specs=[pl.BlockSpec(memory_space=pl.ANY)],
        out_specs=pl.BlockSpec(memory_space=pltpu.VMEM),
        scratch_shapes=[
            pltpu.VMEM(((A + 2) * PITCH, LANE), x.dtype),
            pltpu.VMEM((TILES * SUB, LANE, A), x.dtype),
            pltpu.SemaphoreType.DMA((len(PIECES),)),
            pltpu.SemaphoreType.DMA((2,)),
            pltpu.SemaphoreType.DMA((2,)),
        ],
        compiler_params=pltpu.CompilerParams(vmem_limit_bytes=80 << 20, collective_id=0),
    )(xv)
    k = k.reshape((2,) * 6 + (SUB, LANE, A)).transpose(8, 0, 1, 2, 3, 4, 5, 6, 7)
    return k.reshape(M // SUB, NC, SUB, LANE).transpose(0, 2, 1, 3).reshape(M, N)
```

```python
import jax
import jax.numpy as jnp
from jax import lax
from jax.experimental import pallas as pl
from jax.experimental.pallas import tpu as pltpu

N_DEV = 4
SUB = 8
ROW_BLOCKS, COL_BLOCKS = 4, 2
SLAB = 256
STEP = 64
FIRST_READ = 512
LAST_READS = (2048, 768, 320, 128, 48, 16)
HALO_AFTER = 2


def _read_ranges(m):
    ends = [m - FIRST_READ]
    for rows in reversed(LAST_READS):
        ends.insert(0, ends[0] - rows)
    return [(m - FIRST_READ, m)] + list(zip([0] + ends[:-1], ends))


def _stencil_body(x_hbm, *refs):
    *out_refs, xb, read_sems, send_sems, recv_sems = refs
    m, n = x_hbm.shape
    block_rows, block_cols = m // ROW_BLOCKS, n // COL_BLOCKS
    outs = [o.reshape(block_rows, block_cols) for o in out_refs]

    ranges = _read_ranges(m)
    reads = [
        pltpu.make_async_copy(
            x_hbm.at[pl.ds(lo, hi - lo)], xb.at[pl.ds(SUB + lo, hi - lo)], read_sems.at[i]
        )
        for i, (lo, hi) in enumerate(ranges)
    ]
    for read in reads:
        read.start()

    me = lax.axis_index("i")
    left = (me + N_DEV - 1) % N_DEV
    right = (me + 1) % N_DEV
    barrier = pltpu.get_barrier_semaphore()
    for neighbour in (left, right):
        pl.semaphore_signal(
            barrier, inc=1, device_id=(neighbour,), device_id_type=pl.DeviceIdType.MESH
        )

    def halo_copy(src_row, dst_row, slot, target):
        return pltpu.make_async_remote_copy(
            src_ref=xb.at[pl.ds(src_row, SUB)],
            dst_ref=xb.at[pl.ds(dst_row, SUB)],
            send_sem=send_sems.at[slot],
            recv_sem=recv_sems.at[slot],
            device_id=(target,),
            device_id_type=pl.DeviceIdType.MESH,
        )

    to_left = halo_copy(SUB, SUB + m, 0, left)
    to_right = halo_copy(m, 0, 1, right)

    def stencil(row, rows):
        v = xb[pl.ds(row, rows + 2 * SUB), :]
        quarter = 0.25 * v
        above = pltpu.roll(quarter, 1, 0)[SUB:-SUB]
        below = pltpu.roll(quarter, rows + 2 * SUB - 1, 0)[SUB:-SUB]
        return (above + 0.5 * v[SUB:-SUB]) + below

    def store(block, row, value):
        dst = pl.ds(row - block * block_rows, value.shape[0])
        for c in range(COL_BLOCKS):
            outs[block * COL_BLOCKS + c][dst, :] = value[:, c * block_cols : (c + 1) * block_cols]

    def compute(start, stop):
        for block in range(ROW_BLOCKS):
            lo, hi = max(start, block * block_rows), min(stop, (block + 1) * block_rows)
            steps = (hi - lo) // STEP
            if steps >= 2:

                @pl.loop(0, steps)
                def _(t):
                    row = pl.multiple_of(lo + t * STEP, SUB)
                    store(block, row, stencil(row, STEP))

                lo += steps * STEP
            if hi > lo:
                store(block, lo, stencil(lo, hi - lo))

    for i, (lo, hi) in enumerate(ranges):
        reads[i].wait()
        if i == 0:
            pl.semaphore_wait(barrier, 2)
            to_right.start()
        if i == 1:
            to_left.start()
        compute(lo + SUB if i < 2 else lo - SUB, hi + SUB if i == len(ranges) - 1 else hi - SUB)
        if i == HALO_AFTER:
            to_left.wait_recv()
            to_right.wait_recv()
            sublane = lax.broadcasted_iota(jnp.int32, (SUB, n), 0)
            top_edge = (sublane == 0) & (me == 0)
            bottom_edge = (sublane == SUB - 1) & (me == N_DEV - 1)
            store(0, 0, jnp.where(top_edge, xb[pl.ds(SUB, SUB), :], stencil(0, SUB)))
            store(
                ROW_BLOCKS - 1,
                m - SUB,
                jnp.where(bottom_edge, xb[pl.ds(m, SUB), :], stencil(m - SUB, SUB)),
            )
            to_left.wait_send()
            to_right.wait_send()


def pallas_dist_halo_stencil_i_m8192_n1024_kernel(x: jax.Array):
    m, n = x.shape
    n_blocks = ROW_BLOCKS * COL_BLOCKS
    block = pltpu.VMEM((m // ROW_BLOCKS // SLAB, SLAB, n // COL_BLOCKS), x.dtype)
    blocks = pl.pallas_call(
        _stencil_body,
        out_shape=[block] * n_blocks,
        in_specs=[pl.BlockSpec(memory_space=pl.ANY)],
        out_specs=[pl.BlockSpec(memory_space=pltpu.VMEM)] * n_blocks,
        scratch_shapes=[
            pltpu.VMEM((m + 2 * SUB, n), x.dtype),
            pltpu.SemaphoreType.DMA((len(LAST_READS) + 2,)),
            pltpu.SemaphoreType.DMA((2,)),
            pltpu.SemaphoreType.DMA((2,)),
        ],
        compiler_params=pltpu.CompilerParams(
            vmem_limit_bytes=48 << 20, collective_id=0, disable_semaphore_checks=True
        ),
    )(x)
    rows = [
        jnp.concatenate(blocks[b * COL_BLOCKS : (b + 1) * COL_BLOCKS], axis=2)
        for b in range(ROW_BLOCKS)
    ]
    return jnp.concatenate(rows, axis=0).reshape(m, n)
```

```python
import jax
import jax.numpy as jnp
from jax import lax
from jax.experimental import pallas as pl
from jax.experimental.pallas import tpu as pltpu

N_DEV = 4
SUB = 8
ROW_BLOCKS, COL_BLOCKS = 4, 2
SLAB = 256
STEP = 64
EDGE_READ = 256
LAST_READS = (2048, 768, 320, 128, 48, 16)
N_SLOTS = 4


def _read_ranges(m):
    ends = [m - EDGE_READ]
    for rows in reversed(LAST_READS):
        ends.insert(0, ends[0] - rows)
    return [(m - EDGE_READ, m), (0, EDGE_READ)] + list(zip([EDGE_READ] + ends[:-1], ends))


def _stencil_body(x_hbm, *refs):
    *out_refs, xb, sems, recv_sems = refs
    m, n = x_hbm.shape
    block_rows, block_cols = m // ROW_BLOCKS, n // COL_BLOCKS
    outs = [o.reshape(block_rows, block_cols) for o in out_refs]

    ranges = _read_ranges(m)
    reads = [
        pltpu.make_async_copy(
            x_hbm.at[pl.ds(lo, hi - lo)], xb.at[pl.ds(SUB + lo, hi - lo)], sems.at[i % N_SLOTS]
        )
        for i, (lo, hi) in enumerate(ranges)
    ]
    for read in reads[:N_SLOTS]:
        read.start()

    me = lax.axis_index("i")
    left = (me + N_DEV - 1) % N_DEV
    right = (me + 1) % N_DEV
    barrier = pltpu.get_barrier_semaphore()
    for neighbour in (left, right):
        pl.semaphore_signal(
            barrier, inc=1, device_id=(neighbour,), device_id_type=pl.DeviceIdType.MESH
        )

    def halo_copy(src_row, dst_row, slot, target):
        return pltpu.make_async_remote_copy(
            src_ref=xb.at[pl.ds(src_row, SUB)],
            dst_ref=xb.at[pl.ds(dst_row, SUB)],
            send_sem=sems.at[slot],
            recv_sem=recv_sems.at[slot],
            device_id=(target,),
            device_id_type=pl.DeviceIdType.MESH,
        )

    to_right = halo_copy(m, 0, 0, right)
    to_left = halo_copy(SUB, SUB + m, 1, left)

    def stencil(row, rows):
        v = xb[pl.ds(row, rows + 2 * SUB), :]
        quarter = 0.25 * v
        above = pltpu.roll(quarter, 1, 0)[SUB:-SUB]
        below = pltpu.roll(quarter, rows + 2 * SUB - 1, 0)[SUB:-SUB]
        return (above + 0.5 * v[SUB:-SUB]) + below

    def store(block, row, value):
        dst = pl.ds(row - block * block_rows, value.shape[0])
        for c in range(COL_BLOCKS):
            outs[block * COL_BLOCKS + c][dst, :] = value[:, c * block_cols : (c + 1) * block_cols]

    def compute(start, stop):
        for block in range(ROW_BLOCKS):
            lo, hi = max(start, block * block_rows), min(stop, (block + 1) * block_rows)
            steps = (hi - lo) // STEP
            if steps >= 2:

                @pl.loop(0, steps)
                def _(t):
                    row = pl.multiple_of(lo + t * STEP, SUB)
                    store(block, row, stencil(row, STEP))

                lo += steps * STEP
            if hi > lo:
                store(block, lo, stencil(lo, hi - lo))

    reads[0].wait()
    pl.semaphore_wait(barrier, 2)
    to_right.start()
    reads[1].wait()
    to_left.start()
    compute(m - EDGE_READ + SUB, m - SUB)

    reads[2].wait()
    compute(SUB, ranges[2][1] - SUB)

    to_right.wait()
    to_left.wait()
    for read in reads[N_SLOTS : N_SLOTS + 3]:
        read.start()
    sublane = lax.broadcasted_iota(jnp.int32, (SUB, n), 0)
    first_row = (sublane == 0) & (me == 0)
    last_row = (sublane == SUB - 1) & (me == N_DEV - 1)
    store(0, 0, jnp.where(first_row, xb[pl.ds(SUB, SUB), :], stencil(0, SUB)))
    store(
        ROW_BLOCKS - 1, m - SUB, jnp.where(last_row, xb[pl.ds(m, SUB), :], stencil(m - SUB, SUB))
    )

    for i in range(3, len(reads)):
        lo, hi = ranges[i]
        reads[i].wait()
        if i + N_SLOTS < len(reads):
            reads[i + N_SLOTS].start()
        compute(lo - SUB, hi + SUB if i == len(reads) - 1 else hi - SUB)


def pallas_dist_halo_stencil_i_m8192_n1024_kernel(x: jax.Array):
    m, n = x.shape
    n_blocks = ROW_BLOCKS * COL_BLOCKS
    block = jax.ShapeDtypeStruct((m // ROW_BLOCKS // SLAB, SLAB, n // COL_BLOCKS), x.dtype)
    blocks = pl.pallas_call(
        _stencil_body,
        out_shape=[block] * n_blocks,
        in_specs=[pl.BlockSpec(memory_space=pl.ANY)],
        out_specs=[pl.BlockSpec(memory_space=pltpu.VMEM)] * n_blocks,
        scratch_shapes=[
            pltpu.VMEM((m + 2 * SUB, n), x.dtype),
            pltpu.SemaphoreType.DMA((N_SLOTS,)),
            pltpu.SemaphoreType.DMA((2,)),
        ],
        compiler_params=pltpu.CompilerParams(vmem_limit_bytes=48 << 20, collective_id=0),
    )(x)
    rows = [
        jnp.concatenate(blocks[b * COL_BLOCKS : (b + 1) * COL_BLOCKS], axis=2)
        for b in range(ROW_BLOCKS)
    ]
    return jnp.concatenate(rows, axis=0).reshape(m, n)
```

```python
import jax
import jax.numpy as jnp
from jax import lax
from jax.experimental import pallas as pl
from jax.experimental.pallas import tpu as pltpu

N_DEV = 4
SUB = 8
ROW_BLOCKS, COL_BLOCKS = 4, 2
SLAB = 256
STEP = 64
EDGE = 64
LAST_READS = (2048, 768, 320, 128, 32, 16)
N_SLOTS = 4


def _read_ranges(m):
    top, bottom = EDGE + SUB, m - EDGE - SUB
    ends = [bottom]
    for rows in reversed(LAST_READS):
        ends.insert(0, ends[0] - rows)
    return [(bottom, m), (0, top)] + list(zip([top] + ends[:-1], ends))


def _stencil_body(x_hbm, *refs):
    *outs, xb, sems, recv_sems = refs
    m, n = x_hbm.shape
    block_rows, block_cols = m // ROW_BLOCKS, n // COL_BLOCKS

    ranges = _read_ranges(m)
    reads = [
        pltpu.make_async_copy(
            x_hbm.at[pl.ds(lo, hi - lo)], xb.at[pl.ds(SUB + lo, hi - lo)], sems.at[i % N_SLOTS]
        )
        for i, (lo, hi) in enumerate(ranges)
    ]
    for read in reads[:N_SLOTS]:
        read.start()

    me = lax.axis_index("i")
    left = (me + N_DEV - 1) % N_DEV
    right = (me + 1) % N_DEV
    barrier = pltpu.get_barrier_semaphore()
    for neighbour in (left, right):
        pl.semaphore_signal(
            barrier, inc=1, device_id=(neighbour,), device_id_type=pl.DeviceIdType.MESH
        )

    def halo_copy(src_row, dst_row, slot, target):
        return pltpu.make_async_remote_copy(
            src_ref=xb.at[pl.ds(src_row, SUB)],
            dst_ref=xb.at[pl.ds(dst_row, SUB)],
            send_sem=sems.at[slot],
            recv_sem=recv_sems.at[slot],
            device_id=(target,),
            device_id_type=pl.DeviceIdType.MESH,
        )

    to_right = halo_copy(m, 0, 0, right)
    to_left = halo_copy(SUB, SUB + m, 1, left)

    def stencil(row, rows):
        v = xb[pl.ds(row, rows + 2 * SUB), :]
        quarter = 0.25 * v
        above = pltpu.roll(quarter, 1, 0)[SUB:-SUB]
        below = pltpu.roll(quarter, rows + 2 * SUB - 1, 0)[SUB:-SUB]
        return (above + 0.5 * v[SUB:-SUB]) + below

    def store(block, slab, offset, value):
        for c in range(COL_BLOCKS):
            outs[block * COL_BLOCKS + c][slab, pl.ds(offset, value.shape[0]), :] = value[
                :, c * block_cols : (c + 1) * block_cols
            ]

    def compute(row, stop):
        while row < stop:
            block, slab = divmod(row // SLAB, block_rows // SLAB)
            steps = (min(stop, (block + 1) * block_rows) - row) // STEP
            if row % STEP == 0 and steps >= 2:
                first = row % block_rows // STEP

                @pl.loop(first, first + steps)
                def _(t):
                    src = pl.multiple_of(block * block_rows + t * STEP, STEP)
                    offset = pl.multiple_of(lax.rem(t, SLAB // STEP) * STEP, STEP)
                    store(block, lax.div(t, SLAB // STEP), offset, stencil(src, STEP))

                row += steps * STEP
            else:
                rows = min(stop, (row // STEP + 1) * STEP) - row
                store(block, slab, row % SLAB, stencil(row, rows))
                row += rows

    reads[0].wait()
    pl.semaphore_wait(barrier, 2)
    to_right.start()
    reads[1].wait()
    to_left.start()

    reads[2].wait()
    compute(EDGE, ranges[2][1] - SUB)

    to_right.wait()
    to_left.wait()
    for read in reads[N_SLOTS : N_SLOTS + 3]:
        read.start()
    row_id = lax.broadcasted_iota(jnp.int32, (EDGE, n), 0)
    first_row = (row_id == 0) & (me == 0)
    last_row = (row_id == EDGE - 1) & (me == N_DEV - 1)
    store(0, 0, 0, jnp.where(first_row, xb[pl.ds(SUB, EDGE), :], stencil(0, EDGE)))
    store(
        ROW_BLOCKS - 1,
        block_rows // SLAB - 1,
        SLAB - EDGE,
        jnp.where(last_row, xb[pl.ds(SUB + m - EDGE, EDGE), :], stencil(m - EDGE, EDGE)),
    )

    for i in range(3, len(reads)):
        lo, hi = ranges[i]
        reads[i].wait()
        if i + N_SLOTS < len(reads):
            reads[i + N_SLOTS].start()
        compute(lo - SUB, hi + SUB if i == len(reads) - 1 else hi - SUB)


def pallas_dist_halo_stencil_i_m8192_n1024_kernel(x: jax.Array):
    m, n = x.shape
    n_blocks = ROW_BLOCKS * COL_BLOCKS
    block = jax.ShapeDtypeStruct((m // ROW_BLOCKS // SLAB, SLAB, n // COL_BLOCKS), x.dtype)
    blocks = pl.pallas_call(
        _stencil_body,
        out_shape=[block] * n_blocks,
        in_specs=[pl.BlockSpec(memory_space=pl.ANY)],
        out_specs=[pl.BlockSpec(memory_space=pltpu.VMEM)] * n_blocks,
        scratch_shapes=[
            pltpu.VMEM((m + 2 * SUB, n), x.dtype),
            pltpu.SemaphoreType.DMA((N_SLOTS,)),
            pltpu.SemaphoreType.DMA((2,)),
        ],
        compiler_params=pltpu.CompilerParams(vmem_limit_bytes=72 << 20, collective_id=0),
    )(x)
    rows = [
        jnp.concatenate(blocks[b * COL_BLOCKS : (b + 1) * COL_BLOCKS], axis=2)
        for b in range(ROW_BLOCKS)
    ]
    return jnp.concatenate(rows, axis=0).reshape(m, n)
```
